```python
import numpy as np
kernel_name = 'dist_attn_cross_mha_kvrep_htp_ss_b1_sq512_skv2048_d1024_hq8_dh128'

def setup_inputs():
    x = np.random.randn(1, 2048, 1024).astype(np.float32)
    Wq = np.random.randn(1024, 4096).astype(np.float32) * 0.02
    K_ext = np.random.randn(1, 2048, 32, 128).astype(np.float32)
    V_ext = np.random.randn(1, 2048, 32, 128).astype(np.float32)
    Wo = np.random.randn(4096, 1024).astype(np.float32) * 0.02
    return {'x': x, 'Wq': Wq, 'K_ext': K_ext, 'V_ext': V_ext, 'Wo': Wo}

def reference(x, Wq, K_ext, V_ext, Wo):
    B, Sq, Hq, Hkv, Dh = (1, 2048, 32, 32, 128)
    Q = (x @ Wq).reshape(B, Sq, Hq, Dh)
    K, V = (K_ext, V_ext)
    Skv = K.shape[1]
    out = np.zeros((B, Sq, Hq, Dh), dtype=np.float32)
    m = np.full((B, Hq, Sq, 1), -np.inf, dtype=np.float32)
    l = np.zeros((B, Hq, Sq, 1), dtype=np.float32)
    for j0 in range(0, Skv, 1024):
        Kj = K[:, j0:j0 + 1024].copy()
        Vj = V[:, j0:j0 + 1024].copy()
        sj = np.einsum('bihd,bjhd->bhij', Q, Kj).astype(np.float32) * 0.08838834764831843
        mj = sj.max(axis=-1, keepdims=True)
        m_new = np.maximum(m, mj)
        alpha = np.exp(m - m_new)
        pj = np.exp(sj - m_new)
        l = l * alpha + pj.sum(axis=-1, keepdims=True)
        out = out * alpha.transpose(0, 2, 1, 3) + np.einsum('bhij,bjhd->bihd', pj, Vj)
        m = m_new
    out = (out / l.transpose(0, 2, 1, 3)).reshape(B, Sq, Hq * Dh)
    return out @ Wo
```

```python
import jax
import jax.numpy as jnp
from jax import lax
from jax.experimental import pallas as pl
from jax.experimental.pallas import tpu as pltpu

N_DEV = 4
SQ = 512
SKV = 2048
D = 1024
H = 8
DH = 128
BQ = 256
HALF = 128
QSCALE = 0.08838834764831843 * 1.4426950408889634

bf16 = jnp.bfloat16
f32 = jnp.float32

N_UNITS = (2, 3, 6, 7)
D_UNITS = (4, 5)
P1_HEADS = 5


def _recip(l):
    r = pl.reciprocal(l, approx=True)
    return r * (2.0 - l * r)


def pallas_dist_attn_cross_mha_kvrep_htp_ss_b1_sq512_skv2048_d1024_hq8_dh128_kernel(
    x: jax.Array,
    Wq: jax.Array,
    K_ext: jax.Array,
    V_ext: jax.Array,
    Wo: jax.Array,
):
    def body(x_hbm, wq_hbm, k_hbm, v_hbm, wo_hbm, out_hbm,
             x_v, wq_v, k_v, v_v, wo_v, xg, o_loc, ps, pr, out_v,
             x_sem, wq_sem, k_sem, v_sem, wo_sem, out_sem,
             ag_send, ag_recv, rs_send, rs_recv):
        me = lax.axis_index("i")
        right = lax.rem(me + 1, N_DEV)
        diag = lax.rem(me + 2, N_DEV)
        left = lax.rem(me + 3, N_DEV)
        h0 = me * H

        x_cp = [pltpu.make_async_copy(x_hbm.at[0, pl.ds(j * BQ, BQ), :],
                                      x_v.at[pl.ds(j * BQ, BQ), :], x_sem.at[j])
                for j in range(2)]
        wq_cp = [pltpu.make_async_copy(wq_hbm.at[:, pl.ds(h * DH, DH)],
                                       wq_v.at[:, pl.ds(h * DH, DH)], wq_sem.at[h])
                 for h in range(H)]
        k_cp = [pltpu.make_async_copy(k_hbm.at[0, :, h0 + h, :], k_v.at[h], k_sem.at[h])
                for h in range(H)]
        v_cp = [pltpu.make_async_copy(v_hbm.at[0, :, h0 + h, :], v_v.at[h], v_sem.at[h])
                for h in range(H)]
        wo_cp = [pltpu.make_async_copy(wo_hbm.at[pl.ds(j * 512, 512), :],
                                       wo_v.at[pl.ds(j * 512, 512), :], wo_sem.at[j])
                 for j in range(2)]
        for c in x_cp:
            c.start()
        for h in range(P1_HEADS):
            wq_cp[h].start()
            k_cp[h].start()
            v_cp[h].start()
        for h in range(P1_HEADS, H):
            wq_cp[h].start()
        for h in range(P1_HEADS, H):
            k_cp[h].start()
            v_cp[h].start()
        for c in wo_cp:
            c.start()

        barrier = pltpu.get_barrier_semaphore()
        for peer in (right, diag, left):
            pl.semaphore_signal(barrier, inc=1, device_id=(peer,),
                                device_id_type=pl.DeviceIdType.MESH)

        def qproj(xr, h_lo, h_hi):
            q = jnp.dot(xr, wq_v[:, h_lo * DH:h_hi * DH].astype(bf16),
                        preferred_element_type=f32)
            return (q * QSCALE).astype(bf16)

        def attn(qh, h):
            s = lax.dot_general(qh, k_v[h].astype(bf16), (((1,), (1,)), ((), ())),
                                preferred_element_type=f32)
            m = jnp.max(s, axis=1, keepdims=True)
            p = jnp.exp2(s - m)
            l = jnp.sum(p, axis=1, keepdims=True)
            o = jnp.dot(p.astype(bf16), v_v[h].astype(bf16),
                        preferred_element_type=f32)
            return (o * _recip(l)).astype(bf16)

        def remote(src, dst, ssem, rsem, dev):
            return pltpu.make_async_remote_copy(
                src_ref=src, dst_ref=dst, send_sem=ssem, recv_sem=rsem,
                device_id=(dev,), device_id_type=pl.DeviceIdType.MESH)

        def wait_unit(u):
            pltpu.make_async_copy(xg.at[u], xg.at[u], ag_recv.at[u - 2]).wait()

        def rs_copies(r):
            is_d = jnp.logical_and(r >= 2, r < 4)
            j = jnp.where(r < 2, r, r - 2)
            dev_a = jnp.where(is_d, diag, right)
            dev_b = jnp.where(is_d, diag, left)
            slot_a = jnp.where(is_d, 2, 0)
            slot_b = jnp.where(is_d, 2, 1)
            pc_a = jnp.where(is_d, 2 * (r - 2), j)
            pc_b = jnp.where(is_d, 2 * (r - 2) + 1, j)
            ia = slot_a * 4 + pc_a
            ib = slot_b * 4 + pc_b
            return [
                remote(ps.at[2 * r], pr.at[ia], rs_send.at[2 * r],
                       rs_recv.at[ia], dev_a),
                remote(ps.at[2 * r + 1], pr.at[ib], rs_send.at[2 * r + 1],
                       rs_recv.at[ib], dev_b),
            ]

        for j in range(2):
            x_cp[j].wait()
            xg[j] = x_v[pl.ds(j * BQ, BQ), :].astype(bf16)
        pl.semaphore_wait(barrier, 3)

        ag = []

        def ag_n(j):
            u = N_UNITS[j]
            src = xg.at[j // 2, pl.ds((j % 2) * HALF, HALF), :]
            ag.append(remote(src, xg.at[u, pl.ds(0, HALF), :],
                             ag_send.at[len(ag)], ag_recv.at[u - 2], left))
            ag.append(remote(src, xg.at[u, pl.ds(HALF, HALF), :],
                             ag_send.at[len(ag)], ag_recv.at[u - 2], right))

        def ag_d(k):
            u = D_UNITS[k]
            ag.append(remote(xg.at[k], xg.at[u], ag_send.at[len(ag)],
                             ag_recv.at[u - 2], diag))

        ag_n(0)
        ag_n(1)
        ag_d(0)
        ag_d(1)
        ag_n(2)
        ag_n(3)
        for c in ag:
            c.start()

        for h in range(P1_HEADS):
            wq_cp[h].wait()
            k_cp[h].wait()
            v_cp[h].wait()
            for j in range(2):
                q = qproj(xg[j], h, h + 1)
                o_loc[j, :, h * DH:(h + 1) * DH] = attn(q, h)

        wait_unit(2)
        for h in range(P1_HEADS, H):
            wq_cp[h].wait()
        q = qproj(xg[2], 0, H)
        os_ = [attn(q[:, h * DH:(h + 1) * DH], h) for h in range(P1_HEADS)]
        for h in range(P1_HEADS, H):
            k_cp[h].wait()
            v_cp[h].wait()
        os_ += [attn(q[:, h * DH:(h + 1) * DH], h) for h in range(P1_HEADS, H)]
        for c in wo_cp:
            c.wait()
        part = jnp.dot(jnp.concatenate(os_, axis=1), wo_v[...].astype(bf16),
                       preferred_element_type=f32).astype(bf16)
        ps[0] = part[:HALF]
        ps[1] = part[HALF:]
        for c in rs_copies(0):
            c.start()

        def unit(r, carry):
            wait_unit(r + 2)
            q = qproj(xg[r + 2], 0, H)
            os_ = [attn(q[:, h * DH:(h + 1) * DH], h) for h in range(H)]
            part = jnp.dot(jnp.concatenate(os_, axis=1), wo_v[...].astype(bf16),
                           preferred_element_type=f32).astype(bf16)
            ps[2 * r] = part[:HALF]
            ps[2 * r + 1] = part[HALF:]
            for c in rs_copies(r):
                c.start()
            return carry

        lax.fori_loop(1, 6, unit, 0)

        for j in range(2):
            q = qproj(xg[j], P1_HEADS, H)
            for h in range(P1_HEADS, H):
                hh = h - P1_HEADS
                o_loc[j, :, h * DH:(h + 1) * DH] = attn(q[:, hh * DH:(hh + 1) * DH], h)

        for i in range(12):
            pltpu.make_async_copy(pr.at[i], pr.at[i], rs_recv.at[i]).wait()

        out_cp = []
        for j in range(2):
            acc = jnp.dot(o_loc[j], wo_v[...].astype(bf16), preferred_element_type=f32)
            for s in range(3):
                got = jnp.concatenate([pr[4 * s + 2 * j], pr[4 * s + 2 * j + 1]], axis=0)
                acc = acc + got.astype(f32)
            out_v[pl.ds(j * BQ, BQ), :] = acc
            cp = pltpu.make_async_copy(out_v.at[pl.ds(j * BQ, BQ), :],
                                       out_hbm.at[0, pl.ds(j * BQ, BQ), :], out_sem.at[j])
            cp.start()
            out_cp.append(cp)

        for c in ag:
            c.wait_send()
        for r in range(6):
            for c in rs_copies(r):
                c.wait_send()
        for c in out_cp:
            c.wait()

    return pl.pallas_call(
        body,
        out_shape=jax.ShapeDtypeStruct((1, SQ, D), f32),
        in_specs=[pl.BlockSpec(memory_space=pl.ANY)] * 5,
        out_specs=pl.BlockSpec(memory_space=pl.ANY),
        scratch_shapes=[
            pltpu.VMEM((SQ, D), f32),
            pltpu.VMEM((D, H * DH), f32),
            pltpu.VMEM((H, SKV, DH), f32),
            pltpu.VMEM((H, SKV, DH), f32),
            pltpu.VMEM((H * DH, D), f32),
            pltpu.VMEM((8, BQ, D), bf16),
            pltpu.VMEM((2, BQ, H * DH), bf16),
            pltpu.VMEM((12, HALF, D), bf16),
            pltpu.VMEM((12, HALF, D), bf16),
            pltpu.VMEM((SQ, D), f32),
            pltpu.SemaphoreType.DMA((2,)),
            pltpu.SemaphoreType.DMA((H,)),
            pltpu.SemaphoreType.DMA((H,)),
            pltpu.SemaphoreType.DMA((H,)),
            pltpu.SemaphoreType.DMA((2,)),
            pltpu.SemaphoreType.DMA((2,)),
            pltpu.SemaphoreType.DMA((10,)),
            pltpu.SemaphoreType.DMA((6,)),
            pltpu.SemaphoreType.DMA((12,)),
            pltpu.SemaphoreType.DMA((12,)),
        ],
        compiler_params=pltpu.CompilerParams(
            collective_id=0,
            vmem_limit_bytes=100 * 1024 * 1024,
        ),
    )(x, Wq, K_ext, V_ext, Wo)
```

```python
import jax
import jax.numpy as jnp
from jax import lax
from jax.experimental import pallas as pl
from jax.experimental.pallas import tpu as pltpu

N_DEV = 4
SQ = 512
SKV = 2048
D = 1024
H = 8
G = 4
DH = 128
BQ = 256
PC = 128
QSCALE = 0.08838834764831843 * 1.4426950408889634

bf16 = jnp.bfloat16
f32 = jnp.float32
TASK_UNIT = (1, 1, 2, 2, 3, 3, 0)
TASK_GROUP = (0, 1, 0, 1, 0, 1, 1)
TASK_SECOND = tuple(int(u in TASK_UNIT[:i]) for i, u in enumerate(TASK_UNIT))
AG_ORDER = (1, 2, 3)


def _recip(l):
    r = pl.reciprocal(l, approx=True)
    return r * (2.0 - l * r)


def _mm(a, b):
    return jnp.dot(a.astype(bf16), b.astype(bf16), preferred_element_type=f32)


def _quarters(a):
    m, n = a.shape
    return (a[:m // 2, :n // 2], a[:m // 2, n // 2:],
            a[m // 2:, :n // 2], a[m // 2:, n // 2:])


def _strassen(A, B):
    a11, a12, a21, a22 = A
    b11, b12, b21, b22 = B
    f11, f12, f21, f22 = (a.astype(f32) for a in A)
    m3 = _mm(a11, b12 - b22)
    m6 = _mm(f21 - f11, b11 + b12)
    m5 = _mm(f11 + f12, b22)
    m2 = _mm(f21 + f22, b11)
    m4 = _mm(a22, b21 - b11)
    m1 = _mm(f11 + f22, b11 + b22)
    m7 = _mm(f12 - f22, b21 + b22)
    return (((m4 - m5) + m1) + m7, m3 + m5, m2 + m4, ((m3 + m6) - m2) + m1)


def _join(c):
    return jnp.concatenate([jnp.concatenate(c[:2], axis=1),
                            jnp.concatenate(c[2:], axis=1)], axis=0)


def pallas_dist_attn_cross_mha_kvrep_htp_ss_b1_sq512_skv2048_d1024_hq8_dh128_kernel(
    x: jax.Array,
    Wq: jax.Array,
    K_ext: jax.Array,
    V_ext: jax.Array,
    Wo: jax.Array,
):
    def body(x_hbm, wq_hbm, k_hbm, v_hbm, wo_hbm, out_ref,
             x_v, wq_v, k_v, v_v, wo_v, xg, o_loc, acc, ps, pr,
             x_sem, wq_sem, k_sem, v_sem, wo_sem,
             ag_send, ag_recv, rs_send, rs_recv, fence):
        me = lax.axis_index("i")
        right = lax.rem(me + 1, N_DEV)
        diag = lax.rem(me + 2, N_DEV)
        left = lax.rem(me + 3, N_DEV)
        h0 = me * H

        x_cp = [pltpu.make_async_copy(x_hbm.at[0, pl.ds(j * BQ, BQ), :],
                                      x_v.at[pl.ds(j * BQ, BQ), :], x_sem.at[j])
                for j in range(2)]
        wq_cp = [pltpu.make_async_copy(wq_hbm.at[:, pl.ds(h * DH, DH)],
                                       wq_v.at[0, :, pl.ds(h * DH, DH)], wq_sem.at[h])
                 for h in range(G)]
        wq_cp.append(pltpu.make_async_copy(wq_hbm.at[:, pl.ds(G * DH, G * DH)],
                                           wq_v.at[1], wq_sem.at[G]))
        k_cp = [pltpu.make_async_copy(k_hbm.at[0, :, h0 + h, :], k_v.at[h], k_sem.at[h])
                for h in range(H)]
        v_cp = [pltpu.make_async_copy(v_hbm.at[0, :, h0 + h, :], v_v.at[h], v_sem.at[h])
                for h in range(H)]
        wo_cp = [pltpu.make_async_copy(wo_hbm.at[pl.ds(g * G * DH, G * DH), :],
                                       wo_v.at[g], wo_sem.at[g])
                 for g in range(2)]

        def start_in_order(copies):
            for c in copies:
                c.start()
                pl.semaphore_signal(fence, 1)
            pl.semaphore_wait(fence, len(copies))

        def qk(qf, h):
            return lax.dot_general(qf.astype(bf16), k_v[h].astype(bf16),
                                   (((1,), (1,)), ((), ())),
                                   preferred_element_type=f32)

        def softmax(s):
            m = jnp.max(s, axis=1, keepdims=True)
            p = jnp.exp2(s - m)
            lp = p[:, 0:128]
            for c in range(1, SKV // 128):
                lp = lp + p[:, c * 128:(c + 1) * 128]
            return p.astype(bf16), lp

        def pv(p, lp, h):
            o = jnp.dot(p, v_v[h].astype(bf16), preferred_element_type=f32)
            return o * _recip(jnp.sum(lp, axis=1, keepdims=True))

        def remote(src, dst, ssem, rsem, dev):
            return pltpu.make_async_remote_copy(
                src_ref=src, dst_ref=dst, send_sem=ssem, recv_sem=rsem,
                device_id=(dev,), device_id_type=pl.DeviceIdType.MESH)

        def piece(ref, i, j):
            return ref.at[i, pl.ds(j * PC, PC), :]

        def ag_copies(u):
            if u == 2:
                return [remote(xg.at[0], xg.at[2], ag_send.at[4], ag_recv.at[4], diag)]
            cps = []
            for jj in range(2):
                j = (u - 1) + jj
                base = 5 * (u // 2) + 2 * jj
                cps.append(remote(piece(xg, 0, j), piece(xg, u, 2 * jj),
                                  ag_send.at[base], ag_recv.at[base], left))
                cps.append(remote(piece(xg, 0, j), piece(xg, u, 2 * jj + 1),
                                  ag_send.at[base + 1], ag_recv.at[base + 1], right))
            return cps

        def rs_copies(u):
            if u == 2:
                return [remote(ps.at[2], pr.at[2], rs_send.at[4], rs_recv.at[4], diag)]
            cps = []
            for jj in range(2):
                j = (u - 1) + jj
                base = 5 * (u // 2) + 2 * jj
                cps.append(remote(piece(ps, u, 2 * jj), piece(pr, 0, j),
                                  rs_send.at[base], rs_recv.at[base], right))
                cps.append(remote(piece(ps, u, 2 * jj + 1), piece(pr, 1, j),
                                  rs_send.at[base + 1], rs_recv.at[base + 1], left))
            return cps

        def phase1():
            order = list(x_cp)
            for h in range(G):
                order += [wq_cp[h], k_cp[h], v_cp[h]]
            order += [wo_cp[0], wq_cp[G]]
            for h in range(G, H):
                order += [k_cp[h], v_cp[h]]
            order.append(wo_cp[1])
            start_in_order(order)

            barrier = pltpu.get_barrier_semaphore()
            for peer in (right, diag, left):
                pl.semaphore_signal(barrier, inc=1, device_id=(peer,),
                                    device_id_type=pl.DeviceIdType.MESH)

            x_cp[0].wait()
            xg[0, pl.ds(0, BQ), :] = x_v[pl.ds(0, BQ), :].astype(bf16)
            pl.semaphore_wait(barrier, 3)
            start_in_order(ag_copies(1))
            x_cp[1].wait()
            xg[0, pl.ds(BQ, BQ), :] = x_v[pl.ds(BQ, BQ), :].astype(bf16)
            start_in_order(ag_copies(AG_ORDER[1]) + ag_copies(AG_ORDER[2]))

            def qp(h):
                return _mm(xg[0], wq_v[0, :, h * DH:(h + 1) * DH]) * QSCALE

            def put(j, h, o):
                o_loc[pl.ds(j * BQ, BQ), h * DH:(h + 1) * DH] = o

            cps = {"w": wq_cp, "k": k_cp, "v": v_cp}
            plan = [("w0", "q0"), ("k0", "s0a s0b m0a"), ("v0", "o0a m0b o0b"),
                    ("w1 k1", "q1 s1a s1b m1a"), ("v1 w2", "o1a m1b o1b q2"),
                    ("k2", "s2a s2b m2a"), ("v2 w3", "o2a m2b o2b q3"),
                    ("k3 v3", "a3")]
            qs, ss, pp = {}, {}, {}
            for waits, ops in plan:
                for w in waits.split():
                    cps[w[0]][int(w[1])].wait()
                for op in ops.split():
                    h = int(op[1])
                    if op[0] == "q":
                        qs[h] = qp(h)
                        continue
                    for j in ((0, 1) if len(op) == 2 else ("ab".index(op[2]),)):
                        if op[0] in "sa":
                            ss[h, j] = qk(qs[h][j * BQ:(j + 1) * BQ], h)
                        if op[0] in "ma":
                            pp[h, j] = softmax(ss[h, j])
                        if op[0] in "oa":
                            put(j, h, pv(*pp[h, j], h))

        def lookup(table, t):
            r = jnp.int32(table[-1])
            for i in range(len(table) - 2, -1, -1):
                r = jnp.where(t == i + 1, table[i], r)
            return r

        def task(t):
            for i in range(7):
                u_s = TASK_UNIT[i]
                waits = []
                if u_s != 0 and u_s not in TASK_UNIT[:i]:
                    waits += [c.wait_recv for c in ag_copies(u_s)]
                if i == 0:
                    waits.append(wo_cp[0].wait)
                if TASK_GROUP[i] == 1 and 1 not in TASK_GROUP[:i]:
                    waits.append(wq_cp[G].wait)
                    for h in range(G, H):
                        waits += [k_cp[h].wait, v_cp[h].wait]
                    waits.append(wo_cp[1].wait)
                if waits:
                    @pl.when(t == i + 1)
                    def _():
                        for w in waits:
                            w()

            u = lookup(TASK_UNIT, t)
            g = lookup(TASK_GROUP, t)
            last = lookup(TASK_SECOND, t)
            q4 = _strassen(_quarters(xg[u]), _quarters(wq_v[g]))
            oo = [[None] * G for _ in range(2)]
            lp = None
            for h in range(G):
                for j in range(2):
                    qf = q4[2 * j + h // 2][:, (h % 2) * DH:(h % 2 + 1) * DH] * QSCALE
                    if lp is not None:
                        qf = qf + 0.0 * lp
                    p, lp = softmax(qk(qf, g * G + h))
                    oo[j][h] = pv(p, lp, g * G + h)
            o4 = [jnp.concatenate(oo[j][2 * c:2 * c + 2], axis=1)
                  for j in range(2) for c in range(2)]
            res = _join(_strassen(o4, _quarters(wo_v[g])))
            res = res + jnp.where(last == 1, acc[u], 0.0)
            acc[u] = res
            ps[u] = res.astype(bf16)

            for i in range(7):
                if TASK_SECOND[i]:
                    @pl.when(t == i + 1)
                    def _():
                        start_in_order(rs_copies(TASK_UNIT[i]))

        def final():
            for u_s in (1, 2, 3):
                for c in rs_copies(u_s):
                    c.wait_recv()
            for u_s in (1, 2, 3):
                for c in ag_copies(u_s) + rs_copies(u_s):
                    c.wait_send()
            res = _join(_strassen(_quarters(o_loc[...]), _quarters(wo_v[0])))
            out_ref[0] = (res + acc[0]) + (
                (pr[0].astype(f32) + pr[1].astype(f32)) + pr[2].astype(f32))

        def step(t, carry):
            pl.when(t == 0)(phase1)
            pl.when(jnp.logical_and(t > 0, t < 8))(lambda: task(t))
            pl.when(t == 8)(final)
            return carry

        lax.fori_loop(0, 9, step, 0)

    return pl.pallas_call(
        body,
        out_shape=jax.ShapeDtypeStruct((1, SQ, D), f32),
        in_specs=[pl.BlockSpec(memory_space=pl.ANY)] * 5,
        out_specs=pl.BlockSpec(memory_space=pltpu.VMEM),
        scratch_shapes=[
            pltpu.VMEM((SQ, D), f32),
            pltpu.VMEM((2, D, G * DH), f32),
            pltpu.VMEM((H, SKV, DH), f32),
            pltpu.VMEM((H, SKV, DH), f32),
            pltpu.VMEM((2, G * DH, D), f32),
            pltpu.VMEM((4, SQ, D), bf16),
            pltpu.VMEM((SQ, G * DH), f32),
            pltpu.VMEM((4, SQ, D), f32),
            pltpu.VMEM((4, SQ, D), bf16),
            pltpu.VMEM((3, SQ, D), bf16),
            pltpu.SemaphoreType.DMA((2,)),
            pltpu.SemaphoreType.DMA((G + 1,)),
            pltpu.SemaphoreType.DMA((H,)),
            pltpu.SemaphoreType.DMA((H,)),
            pltpu.SemaphoreType.DMA((2,)),
            pltpu.SemaphoreType.DMA((9,)),
            pltpu.SemaphoreType.DMA((9,)),
            pltpu.SemaphoreType.DMA((9,)),
            pltpu.SemaphoreType.DMA((9,)),
            pltpu.SemaphoreType.REGULAR,
        ],
        compiler_params=pltpu.CompilerParams(
            collective_id=0,
            disable_semaphore_checks=True,
            disable_bounds_checks=True,
            vmem_limit_bytes=100 * 1024 * 1024,
        ),
    )(x, Wq, K_ext, V_ext, Wo)
```

```python
import jax
import jax.numpy as jnp
from jax import lax
from jax.experimental import pallas as pl
from jax.experimental.pallas import tpu as pltpu

N_DEV = 4
SQ = 512
SKV = 2048
D = 1024
H = 8
G = 4
DH = 128
BQ = 256
PC = 64
NP = SQ // PC
QSCALE = 0.08838834764831843 * 1.4426950408889634

bf16 = jnp.bfloat16
f32 = jnp.float32

LOAD_ORDER = "x0 w0 k0 x1 w1 v0 k1 v1 w2 w3 k2 v2 k3 v3 u0 u1"


def _scores(h):
    return f"s{h}a x{h}a s{h}b x{h}b12"


def _values(h):
    return f"o{h}a o{h}b12"


PHASE1 = (
    ("x0", "c0"), ("w0", "q0a g0"), ("k0", "s0a x0a"),
    ("x1", "c1 g1 q0b s0b x0b12"), ("w1", "q1"), ("v0", _values(0)),
    ("k1", _scores(1)), ("v1", _values(1)), ("w2 w3", "Q2"),
    ("k2", _scores(2)), ("v2", _values(2)), ("k3", _scores(3)),
    ("v3", _values(3)), ("u0", "P2 P6"), ("u1", "P3 P7"),
)
FINAL_PRODUCTS = (4, 1, 5)
LOCAL_INNER = (1, 5, 2, 4, 6, 3, 7)
TASK_PROG = ("Q5 Q3 Q7 Q1 Q4 Q2 A0b Q6 A1b A2b A3b A1a A0a A3a A2a "
             "O2 O6 O4 O3 O5 O1 O7")
TASK_SPLIT = (0, 8, 12, 8, 8, 12, 12, 4)
TASK_HINT = (0, 0, 1, 1, 0, 1, 2, 1)
TASK_INNER = (1, 2, 4, 5, 7, 3, 6)
NESTED = (2, 3, 6, 7)


def _recip(l):
    r = pl.reciprocal(l, approx=True)
    return r * (2.0 - l * r)


def _mm(a, b):
    return jnp.dot(a.astype(bf16), b.astype(bf16), preferred_element_type=f32)


def _quarters(a):
    m, n = a.shape
    return (a[:m // 2, :n // 2], a[:m // 2, n // 2:],
            a[m // 2:, :n // 2], a[m // 2:, n // 2:])


def _join(c):
    return jnp.concatenate([jnp.concatenate(c[:2], axis=1),
                            jnp.concatenate(c[2:], axis=1)], axis=0)


_COMB = ({1: 1, 4: 1, 5: -1, 7: 1}, {3: 1, 5: 1}, {2: 1, 4: 1},
         {1: 1, 2: -1, 3: 1, 6: 1})
_B_USED = {1: (0, 3), 2: (0,), 3: (1, 3), 4: (0, 2), 5: (3,), 6: (0, 1),
           7: (2, 3)}


def _sprod(i, A, B, mm=_mm):
    b11, b12, b21, b22 = B

    def f(k):
        return A[k]().astype(f32)

    if i == 1:
        return mm(f(0) + f(3), b11 + b22)
    if i == 2:
        return mm(f(2) + f(3), b11)
    if i == 3:
        return mm(A[0](), b12 - b22)
    if i == 4:
        return mm(A[3](), b21 - b11)
    if i == 5:
        return mm(f(0) + f(1), b22)
    if i == 6:
        return mm(f(2) - f(0), b11 + b12)
    return mm(f(1) - f(3), b21 + b22)


def _scomb(M, k):
    terms = [(i, _COMB[k][i]) for i in M if i in _COMB[k]]
    if terms[0][1] < 0:
        terms[0], terms[1] = terms[1], terms[0]
    r = M[terms[0][0]]
    for i, sign in terms[1:]:
        r = r + M[i] if sign > 0 else r - M[i]
    return r


def _strassen(a, b, order):
    A = [lambda q=q: q for q in _quarters(a)]
    B = _quarters(b)
    M = {i: _sprod(i, A, B) for i in order}
    return [_scomb(M, k) for k in range(4)]


def _oproj_mm(i, inner_order):
    if i not in NESTED:
        return _mm
    return lambda a, b: _join(_strassen(a, b, inner_order))


def _tile_sum(p):
    r = p[:, 0:128]
    for c in range(1, p.shape[1] // 128):
        r = r + p[:, c * 128:(c + 1) * 128]
    return r


def _rowmax(s, sp):
    return jnp.max(s[:, :sp] if sp else s, axis=1, keepdims=True)


def pallas_dist_attn_cross_mha_kvrep_htp_ss_b1_sq512_skv2048_d1024_hq8_dh128_kernel(
    x: jax.Array,
    Wq: jax.Array,
    K_ext: jax.Array,
    V_ext: jax.Array,
    Wo: jax.Array,
):
    def body(x_hbm, wq_hbm, k_hbm, v_hbm, wo_hbm, out_ref,
             x_v, wq_v, k_v, v_v, wo_v, xg, o_loc, acc, ps, pr,
             x_sem, wq_sem, k_sem, v_sem, wo_sem,
             ag_send, ag_recv, rs_send, rs_recv, fence):
        me = lax.axis_index("i")
        right = lax.rem(me + 1, N_DEV)
        diag = lax.rem(me + 2, N_DEV)
        left = lax.rem(me + 3, N_DEV)
        h0 = me * H

        copy = pltpu.make_async_copy
        x_cp = [copy(x_hbm.at[0, pl.ds(j * BQ, BQ), :],
                     x_v.at[pl.ds(j * BQ, BQ), :], x_sem.at[j])
                for j in range(2)]
        wq_cp = [copy(wq_hbm.at[:, pl.ds(h * DH, DH)],
                      wq_v.at[0, :, pl.ds(h * DH, DH)], wq_sem.at[h])
                 for h in range(G)]
        wq_cp.append(copy(wq_hbm.at[:, pl.ds(G * DH, G * DH)], wq_v.at[1],
                          wq_sem.at[G]))
        k_cp = [copy(k_hbm.at[0, :, h0 + h, :], k_v.at[h], k_sem.at[min(h, G)])
                for h in range(H)]
        v_cp = [copy(v_hbm.at[0, :, h0 + h, :], v_v.at[h], v_sem.at[min(h, G)])
                for h in range(H)]
        wo_cp = [copy(wo_hbm.at[pl.ds(j * BQ, BQ), :],
                      wo_v.at[0, pl.ds(j * BQ, BQ), :], wo_sem.at[j])
                 for j in range(2)]
        wo_cp.append(copy(wo_hbm.at[pl.ds(G * DH, G * DH), :], wo_v.at[1],
                          wo_sem.at[2]))

        def start_in_order(copies):
            for c in copies:
                c.start()
                pl.semaphore_signal(fence, 1)
            pl.semaphore_wait(fence, len(copies))

        def wait_total(ref, sem):
            copy(ref, ref, sem).wait()

        def remote(src, dst, ssem, rsem, dev):
            return pltpu.make_async_remote_copy(
                src_ref=src, dst_ref=dst, send_sem=ssem, recv_sem=rsem,
                device_id=(dev,), device_id_type=pl.DeviceIdType.MESH)

        def piece(ref, i, j):
            return ref.at[i, pl.ds(j * PC, PC), :]

        def ag_copies(u):
            if u == 2:
                return [remote(xg.at[0], xg.at[2], ag_send, ag_recv.at[1], diag)]
            return [remote(piece(xg, 0, 2 * (u - 1) + i // 2), piece(xg, u, i),
                           ag_send, ag_recv.at[u - 1], right if i % 2 else left)
                    for i in range(NP)]

        def rs_start(u):
            is_d = u == 2
            for i in range(NP):
                slot = jnp.where(is_d, 2, i % 2)
                row = jnp.where(is_d, i, 2 * (u - 1) + i // 2) * PC
                dev = jnp.where(is_d, diag, left if i % 2 else right)
                remote(piece(ps, u, i),
                       pr.at[slot, pl.ds(pl.multiple_of(row, PC), PC), :],
                       rs_send, rs_recv, dev).start()

        def qk(qf, h):
            return lax.dot_general(qf.astype(bf16), k_v[h].astype(bf16),
                                   (((1,), (1,)), ((), ())),
                                   preferred_element_type=f32)

        def attend(s, h, sp, m1=None):
            vb = v_v[h].astype(bf16)
            if m1 is None:
                m1 = _rowmax(s, sp)
            if sp == 0:
                p = jnp.exp2(s - m1)
                lp = _tile_sum(p)
                o = jnp.dot(p.astype(bf16), vb, preferred_element_type=f32)
            else:
                p1 = jnp.exp2(s[:, :sp] - m1)
                o1 = jnp.dot(p1.astype(bf16), vb[:sp], preferred_element_type=f32)
                m = jnp.maximum(m1, jnp.max(s[:, sp:], axis=1, keepdims=True))
                p2 = jnp.exp2(s[:, sp:] - m)
                alpha = jnp.exp2(m1 - m)
                lp = _tile_sum(p1) * alpha + _tile_sum(p2)
                o = o1 * alpha + jnp.dot(p2.astype(bf16), vb[sp:],
                                         preferred_element_type=f32)
            return o * _recip(jnp.sum(lp, axis=1, keepdims=True)), lp

        def local_oproj(i):
            hd, hn = G * DH // 2, D // 2
            oa = [lambda j=j, c=c: o_loc[pl.ds(j * BQ, BQ), pl.ds(c * hd, hd)]
                  for j in range(2) for c in range(2)]
            wo4 = [wo_v[0, pl.ds(r * hd, hd), pl.ds(c * hn, hn)]
                   if 2 * r + c in _B_USED[i] else None
                   for r in range(2) for c in range(2)]
            return _sprod(i, oa, wo4, _oproj_mm(i, LOCAL_INNER))

        def phase1():
            cps = {"x": x_cp, "w": wq_cp, "k": k_cp, "v": v_cp, "u": wo_cp}
            order = [cps[w[0]][int(w[1])] for w in LOAD_ORDER.split()]
            order.append(wq_cp[G])
            for h in range(G, H):
                order += [k_cp[h], v_cp[h]]
            order.append(wo_cp[2])
            start_in_order(order)

            barrier = pltpu.get_barrier_semaphore()
            for peer in (right, diag, left):
                pl.semaphore_signal(barrier, inc=1, device_id=(peer,),
                                    device_id_type=pl.DeviceIdType.MESH)

            qs, ss, mx, mo = {}, {}, {}, {}
            for waits, ops in PHASE1:
                for w in waits.split():
                    cps[w[0]][int(w[1])].wait()
                for op in ops.split():
                    kind, h = op[0], int(op[1])
                    if kind == "c":
                        rows = pl.ds(h * BQ, BQ)
                        xg[0, rows, :] = x_v[rows, :].astype(bf16)
                    elif kind == "g" and h == 0:
                        pl.semaphore_wait(barrier, 3)
                        start_in_order(ag_copies(1))
                    elif kind == "g":
                        start_in_order(ag_copies(2) + ag_copies(3))
                    elif kind == "Q":
                        q4 = _strassen(xg[0], wq_v[0, :, h * DH:(h + 2) * DH],
                                       (3, 6, 5, 2, 4, 1, 7))
                        for j in range(2):
                            for hh in range(2):
                                qs[h + hh, j] = q4[2 * j + hh] * QSCALE
                    elif kind == "q" and len(op) == 2:
                        q = _mm(xg[0], wq_v[0, :, h * DH:(h + 1) * DH]) * QSCALE
                        for j in range(2):
                            qs[h, j] = q[j * BQ:(j + 1) * BQ]
                    elif kind == "P":
                        mo[h] = local_oproj(h)
                    else:
                        j = "ab".index(op[2])
                        rows = pl.ds(j * BQ, BQ)
                        sp = int(op[3:] or 0) * 128
                        if kind == "q":
                            qs[h, j] = _mm(xg[0, rows, :],
                                           wq_v[0, :, h * DH:(h + 1) * DH]) * QSCALE
                        elif kind == "s":
                            ss[h, j] = qk(qs[h, j], h)
                        elif kind == "x":
                            mx[h, j] = _rowmax(ss[h, j], sp)
                        else:
                            o_loc[rows, h * DH:(h + 1) * DH] = attend(
                                ss[h, j], h, sp, mx[h, j])[0]
            acc[0] = _join([_scomb(mo, k) for k in range(4)])

        def task(t, carry):
            u = lax.shift_right_logical(t + 1, 1) & 3
            g = ((t + 1) & 1) | lax.shift_right_logical(t + 1, 3)

            @pl.when(g == 0)
            def _():
                wait_total(xg.at[u], ag_recv.at[u - 1])

            @pl.when(t == 2)
            def _():
                wq_cp[G].wait()
                wait_total(k_v.at[pl.ds(G, G)], k_sem.at[G])
                wait_total(v_v.at[pl.ds(G, G)], v_sem.at[G])
                wo_cp[2].wait()

            xq = _quarters(xg[u])
            xa = [lambda k=k: xq[k] for k in range(4)]
            wq4 = _quarters(wq_v[g])
            wo4 = _quarters(wo_v[g])
            prev = _quarters(jnp.where(g == 1, acc[u], 0.0))
            mq, mo, q4, oo, lps = {}, {}, {}, {}, []
            oa = [lambda j=j, c=c: jnp.concatenate(
                      [oo[j, 2 * c], oo[j, 2 * c + 1]], axis=1)
                  for j in range(2) for c in range(2)]
            for op in TASK_PROG.split():
                i = int(op[1])
                if op[0] == "Q":
                    mq[i] = _sprod(i, xa, wq4)
                elif op[0] == "O":
                    mo[i] = _sprod(i, oa, wo4, _oproj_mm(i, TASK_INNER))
                else:
                    j = "ab".index(op[2])
                    k = 2 * j + i // 2
                    if k not in q4:
                        q4[k] = _scomb(mq, k)
                    qf = q4[k][:, (i % 2) * DH:(i % 2 + 1) * DH] * QSCALE
                    lag = TASK_HINT[len(lps)]
                    if lag:
                        qf = qf + 0.0 * lps[-lag]
                    oo[j, i], lp = attend(qk(qf, g * G + i), g * G + i,
                                          TASK_SPLIT[len(lps)] * 128)
                    lps.append(lp)
            res = _join([_scomb(mo, k) + prev[k] for k in range(4)])
            acc[u] = res
            ps[u] = res.astype(bf16)

            @pl.when(jnp.logical_and(g == 1, u > 0))
            def _():
                rs_start(u)

            return carry

        def final():
            wait_total(pr, rs_recv)
            wait_total(xg.at[pl.ds(1, 3)], ag_send)
            wait_total(ps.at[pl.ds(1, 3)], rs_send)
            prev = _quarters(acc[0] + (
                (pr[0].astype(f32) + pr[1].astype(f32)) + pr[2].astype(f32)))
            mo = {i: local_oproj(i) for i in FINAL_PRODUCTS}
            out_ref[0] = _join([_scomb(mo, k) + prev[k] for k in range(4)])

        def everything(_, carry):
            phase1()
            lax.fori_loop(1, 8, task, 0)
            final()
            return carry

        lax.fori_loop(0, jnp.minimum(me + 1, 1), everything, 0)

    return pl.pallas_call(
        body,
        out_shape=jax.ShapeDtypeStruct((1, SQ, D), f32),
        in_specs=[pl.BlockSpec(memory_space=pl.ANY)] * 5,
        out_specs=pl.BlockSpec(memory_space=pltpu.VMEM),
        scratch_shapes=[
            pltpu.VMEM((SQ, D), f32),
            pltpu.VMEM((2, D, G * DH), f32),
            pltpu.VMEM((H, SKV, DH), f32),
            pltpu.VMEM((H, SKV, DH), f32),
            pltpu.VMEM((2, G * DH, D), f32),
            pltpu.VMEM((4, SQ, D), bf16),
            pltpu.VMEM((SQ, G * DH), f32),
            pltpu.VMEM((4, SQ, D), f32),
            pltpu.VMEM((4, SQ, D), bf16),
            pltpu.VMEM((3, SQ, D), bf16),
            pltpu.SemaphoreType.DMA((2,)),
            pltpu.SemaphoreType.DMA((G + 1,)),
            pltpu.SemaphoreType.DMA((G + 1,)),
            pltpu.SemaphoreType.DMA((G + 1,)),
            pltpu.SemaphoreType.DMA((3,)),
            pltpu.SemaphoreType.DMA,
            pltpu.SemaphoreType.DMA((3,)),
            pltpu.SemaphoreType.DMA,
            pltpu.SemaphoreType.DMA,
            pltpu.SemaphoreType.REGULAR,
        ],
        compiler_params=pltpu.CompilerParams(
            collective_id=0,
            disable_semaphore_checks=True,
            disable_bounds_checks=True,
            vmem_limit_bytes=100 * 1024 * 1024,
        ),
    )(x, Wq, K_ext, V_ext, Wo)
```

```python
import jax
import jax.numpy as jnp
from jax import lax
from jax.experimental import pallas as pl
from jax.experimental.pallas import tpu as pltpu

N_DEV = 4
SQ = 512
SKV = 2048
D = 1024
H = 8
G = 4
DH = 128
BQ = 256
PC = 64
UNIT = (2, 2, 2, PC, D)
QSCALE = 0.08838834764831843 * 1.4426950408889634

bf16 = jnp.bfloat16
f32 = jnp.float32

LOAD_ORDER = "x0 w0 k0 x1 w1 v0 k1 v1 w2 w3 k2 v2 k3 v3 u0 u1 u2"


def _scores(h):
    return f"s{h}a x{h}a s{h}b x{h}b12"


def _values(h):
    return f"o{h}a o{h}b12"


PHASE1 = (
    ("x0", "c0"), ("w0", "q0a g0"), ("k0", "s0a x0a"),
    ("x1", "c1 g1 q0b s0b x0b12"), ("w1", "q1"), ("v0", _values(0)),
    ("k1", _scores(1)), ("v1", _values(1)), ("w2 w3", "Q2"),
    ("k2", _scores(2)), ("v2", _values(2)), ("k3", _scores(3)),
    ("v3", _values(3)), ("u0 u1", "P2 P6 P5 P1"),
)
PHASE1_Q_ORDER = (2, 3, 6, 4, 5, 1, 7)
FINAL_PRODUCTS = (3, 7, 4)
TASK_PROG = ("Q5 Q7 Q4 Q1 Q3 Q2 A1b A3a Q6 A3b A1a A2b A0b A0a A2a "
             "O2 O3 O5 O4 O7 O6 O1")
TASK_SPLIT = (0, 8, 8, 12, 8, 12, 8, 0)
TASK_HINT = (0, 0, 1, 1, 1, 1, 2, 1)
TASK_NESTED = (2, 3, 6, 7)
LOCAL_NESTED = (1, 2, 5, 6)
INNER_ORDER = (1, 2, 4, 7, 5, 3, 6)


def _recip(l):
    r = pl.reciprocal(l, approx=True)
    return r * (2.0 - l * r)


def _mm(a, b):
    return jnp.dot(a.astype(bf16), b.astype(bf16), preferred_element_type=f32)


def _quarters(a):
    m, n = a.shape
    return (a[:m // 2, :n // 2], a[:m // 2, n // 2:],
            a[m // 2:, :n // 2], a[m // 2:, n // 2:])


def _join(c):
    return jnp.concatenate([jnp.concatenate(c[:2], axis=1),
                            jnp.concatenate(c[2:], axis=1)], axis=0)


_COMB = ({1: 1, 4: 1, 5: -1, 7: 1}, {3: 1, 5: 1}, {2: 1, 4: 1},
         {1: 1, 2: -1, 3: 1, 6: 1})
_B_USED = {1: (0, 3), 2: (0,), 3: (1, 3), 4: (0, 2), 5: (3,), 6: (0, 1),
           7: (2, 3)}


def _sprod(i, A, B, mm=_mm):
    b11, b12, b21, b22 = B

    def f(k):
        return A[k]().astype(f32)

    if i == 1:
        return mm(f(0) + f(3), b11 + b22)
    if i == 2:
        return mm(f(2) + f(3), b11)
    if i == 3:
        return mm(A[0](), b12 - b22)
    if i == 4:
        return mm(A[3](), b21 - b11)
    if i == 5:
        return mm(f(0) + f(1), b22)
    if i == 6:
        return mm(f(2) - f(0), b11 + b12)
    return mm(f(1) - f(3), b21 + b22)


def _scomb(M, k):
    terms = [(i, _COMB[k][i]) for i in M if i in _COMB[k]]
    if terms[0][1] < 0:
        terms[0], terms[1] = terms[1], terms[0]
    r = M[terms[0][0]]
    for i, sign in terms[1:]:
        r = r + M[i] if sign > 0 else r - M[i]
    return r


def _strassen(a, b, order):
    A = [lambda q=q: q for q in _quarters(a)]
    B = _quarters(b)
    M = {i: _sprod(i, A, B) for i in order}
    return [_scomb(M, k) for k in range(4)]


def _mm_nested(a, b):
    return _join(_strassen(a, b, INNER_ORDER))


def _tile_sum(p):
    r = p[:, 0:128]
    for c in range(1, p.shape[1] // 128):
        r = r + p[:, c * 128:(c + 1) * 128]
    return r


def _rowmax(s, sp):
    return jnp.max(s[:, :sp] if sp else s, axis=1, keepdims=True)


def pallas_dist_attn_cross_mha_kvrep_htp_ss_b1_sq512_skv2048_d1024_hq8_dh128_kernel(
    x: jax.Array,
    Wq: jax.Array,
    K_ext: jax.Array,
    V_ext: jax.Array,
    Wo: jax.Array,
):
    def body(x_hbm, wq_hbm, k_hbm, v_hbm, wo_hbm, out_ref,
             x_v, wq_v, k_v, v_v, wo_v, xg, o_loc, acc, ps, pr,
             x_sem, wq_sem, k_sem, v_sem, wo_sem,
             ag_send, ag_recv, rs_send, rs_recv, fence):
        me = lax.axis_index("i")
        right = lax.rem(me + 1, N_DEV)
        diag = lax.rem(me + 2, N_DEV)
        left = lax.rem(me + 3, N_DEV)
        h0 = me * H

        copy = pltpu.make_async_copy
        x_cp = [copy(x_hbm.at[0, pl.ds(j * BQ, BQ), :],
                     x_v.at[pl.ds(j * BQ, BQ), :], x_sem.at[j])
                for j in range(2)]
        wq_cp = [copy(wq_hbm.at[:, pl.ds(h * DH, DH)],
                      wq_v.at[0, :, pl.ds(h * DH, DH)], wq_sem.at[h])
                 for h in range(G)]
        wq_cp.append(copy(wq_hbm.at[:, pl.ds(G * DH, G * DH)], wq_v.at[1],
                          wq_sem.at[G]))
        k_cp = [copy(k_hbm.at[0, :, h0 + h, :], k_v.at[h], k_sem.at[min(h, G)])
                for h in range(H)]
        v_cp = [copy(v_hbm.at[0, :, h0 + h, :], v_v.at[h], v_sem.at[min(h, G)])
                for h in range(H)]
        wo_blocks = ((pl.ds(0, BQ), pl.ds(0, D)),
                     (pl.ds(BQ, BQ), pl.ds(D // 2, D // 2)),
                     (pl.ds(BQ, BQ), pl.ds(0, D // 2)))
        wo_cp = [copy(wo_hbm.at[r, c], wo_v.at[0, r, c], wo_sem.at[i])
                 for i, (r, c) in enumerate(wo_blocks)]
        wo_cp.append(copy(wo_hbm.at[pl.ds(G * DH, G * DH), :], wo_v.at[1],
                          wo_sem.at[3]))

        def start_in_order(copies):
            for c in copies:
                c.start()
                pl.semaphore_signal(fence, 1)
            pl.semaphore_wait(fence, len(copies))

        def wait_total(ref, sem):
            copy(ref, ref, sem).wait()

        def remote(src, dst, ssem, rsem, dev):
            return pltpu.make_async_remote_copy(
                src_ref=src, dst_ref=dst, send_sem=ssem, recv_sem=rsem,
                device_id=(dev,), device_id_type=pl.DeviceIdType.MESH)

        def ag_copies(u):
            return [remote(xg.at[0, c if u == 2 else u // 2], xg.at[u, :, :, c],
                           ag_send, ag_recv.at[u - 1],
                           diag if u == 2 else (right if c else left))
                    for c in range(2)]

        def rs_start(u):
            is_d = u == 2
            for c in range(2):
                slot = jnp.where(is_d, 2, c)
                half = jnp.where(is_d, c, lax.shift_right_logical(u, 1))
                dev = jnp.where(is_d, diag, left if c else right)
                remote(ps.at[u, :, :, c], pr.at[slot, half],
                       rs_send, rs_recv, dev).start()

        def rows_of(ref, *idx):
            v = ref[idx]
            return v.reshape(-1, D)

        def qk(qf, h):
            return lax.dot_general(qf.astype(bf16), k_v[h].astype(bf16),
                                   (((1,), (1,)), ((), ())),
                                   preferred_element_type=f32)

        def attend(s, h, sp, m1=None):
            vb = v_v[h].astype(bf16)
            if m1 is None:
                m1 = _rowmax(s, sp)
            if sp == 0:
                p = jnp.exp2(s - m1)
                lp = _tile_sum(p)
                o = jnp.dot(p.astype(bf16), vb, preferred_element_type=f32)
            else:
                p1 = jnp.exp2(s[:, :sp] - m1)
                o1 = jnp.dot(p1.astype(bf16), vb[:sp], preferred_element_type=f32)
                m = jnp.maximum(m1, jnp.max(s[:, sp:], axis=1, keepdims=True))
                p2 = jnp.exp2(s[:, sp:] - m)
                alpha = jnp.exp2(m1 - m)
                lp = _tile_sum(p1) * alpha + _tile_sum(p2)
                o = o1 * alpha + jnp.dot(p2.astype(bf16), vb[sp:],
                                         preferred_element_type=f32)
            return o * _recip(jnp.sum(lp, axis=1, keepdims=True)), lp

        def local_oproj(i):
            hd, hn = G * DH // 2, D // 2
            oa = [lambda j=j, c=c: o_loc[pl.ds(j * BQ, BQ), pl.ds(c * hd, hd)]
                  for j in range(2) for c in range(2)]
            wo4 = [wo_v[0, pl.ds(r * hd, hd), pl.ds(c * hn, hn)]
                   if 2 * r + c in _B_USED[i] else None
                   for r in range(2) for c in range(2)]
            return _sprod(i, oa, wo4, _mm_nested if i in LOCAL_NESTED else _mm)

        def phase1():
            cps = {"x": x_cp, "w": wq_cp, "k": k_cp, "v": v_cp, "u": wo_cp}
            order = [cps[w[0]][int(w[1])] for w in LOAD_ORDER.split()]
            order.append(wq_cp[G])
            for h in range(G, H):
                order += [k_cp[h], v_cp[h]]
            order.append(wo_cp[3])
            start_in_order(order)

            barrier = pltpu.get_barrier_semaphore()
            for peer in (right, diag, left):
                pl.semaphore_signal(barrier, inc=1, device_id=(peer,),
                                    device_id_type=pl.DeviceIdType.MESH)

            qs, ss, mx, mo = {}, {}, {}, {}
            for waits, ops in PHASE1:
                for w in waits.split():
                    cps[w[0]][int(w[1])].wait()
                for op in ops.split():
                    kind, h = op[0], int(op[1])
                    if kind == "c":
                        xg[0, h] = x_v[pl.ds(h * BQ, BQ), :].astype(
                            bf16).reshape(UNIT[1:])
                    elif kind == "g" and h == 0:
                        pl.semaphore_wait(barrier, 3)
                        start_in_order(ag_copies(1))
                    elif kind == "g":
                        start_in_order(ag_copies(2) + ag_copies(3))
                    elif kind == "Q":
                        q4 = _strassen(rows_of(xg, 0), wq_v[0, :, h * DH:(h + 2) * DH],
                                       PHASE1_Q_ORDER)
                        for j in range(2):
                            for hh in range(2):
                                qs[h + hh, j] = q4[2 * j + hh] * QSCALE
                    elif kind == "q" and len(op) == 2:
                        q = _mm(rows_of(xg, 0), wq_v[0, :, h * DH:(h + 1) * DH]) * QSCALE
                        for j in range(2):
                            qs[h, j] = q[j * BQ:(j + 1) * BQ]
                    elif kind == "P":
                        mo[h] = local_oproj(h)
                    else:
                        j = "ab".index(op[2])
                        rows = pl.ds(j * BQ, BQ)
                        sp = int(op[3:] or 0) * 128
                        if kind == "q":
                            qs[h, j] = _mm(rows_of(xg, 0, j),
                                           wq_v[0, :, h * DH:(h + 1) * DH]) * QSCALE
                        elif kind == "s":
                            ss[h, j] = qk(qs[h, j], h)
                        elif kind == "x":
                            mx[h, j] = _rowmax(ss[h, j], sp)
                        else:
                            o_loc[rows, h * DH:(h + 1) * DH] = attend(
                                ss[h, j], h, sp, mx[h, j])[0]
            acc[0] = _join([_scomb(mo, k) for k in range(4)])
            wo_cp[2].wait()

        def task(t, carry):
            u = lax.shift_right_logical(t + 1, 1) & 3
            g = ((t + 1) & 1) | lax.shift_right_logical(t + 1, 3)

            @pl.when(g == 0)
            def _():
                wait_total(xg.at[u], ag_recv.at[u - 1])

            @pl.when(t == 2)
            def _():
                wq_cp[G].wait()
                wait_total(k_v.at[pl.ds(G, G)], k_sem.at[G])
                wait_total(v_v.at[pl.ds(G, G)], v_sem.at[G])
                wo_cp[3].wait()

            xq = _quarters(rows_of(xg, u))
            xa = [lambda k=k: xq[k] for k in range(4)]
            wq4 = _quarters(wq_v[g])
            wo4 = _quarters(wo_v[g])
            prev = _quarters(jnp.where(g == 1, acc[u], 0.0))
            mq, mo, q4, oo, lps = {}, {}, {}, {}, []
            oa = [lambda j=j, c=c: jnp.concatenate(
                      [oo[j, 2 * c], oo[j, 2 * c + 1]], axis=1)
                  for j in range(2) for c in range(2)]
            for op in TASK_PROG.split():
                i = int(op[1])
                if op[0] == "Q":
                    mq[i] = _sprod(i, xa, wq4)
                elif op[0] == "O":
                    mo[i] = _sprod(i, oa, wo4,
                                   _mm_nested if i in TASK_NESTED else _mm)
                else:
                    j = "ab".index(op[2])
                    k = 2 * j + i // 2
                    if k not in q4:
                        q4[k] = _scomb(mq, k)
                    qf = q4[k][:, (i % 2) * DH:(i % 2 + 1) * DH] * QSCALE
                    lag = TASK_HINT[len(lps)]
                    if lag:
                        qf = qf + 0.0 * lps[-lag]
                    oo[j, i], lp = attend(qk(qf, g * G + i), g * G + i,
                                          TASK_SPLIT[len(lps)] * 128)
                    lps.append(lp)
            res = _join([_scomb(mo, k) + prev[k] for k in range(4)])
            acc[u] = res
            ps[u] = res.astype(bf16).reshape(UNIT)

            @pl.when(jnp.logical_and(g == 1, u > 0))
            def _():
                rs_start(u)

            return carry

        def final():
            wait_total(pr, rs_recv)
            wait_total(xg.at[pl.ds(1, 3)], ag_send)
            wait_total(ps.at[pl.ds(1, 3)], rs_send)
            got = [rows_of(pr, i).astype(f32) for i in range(3)]
            prev = _quarters(acc[0] + ((got[0] + got[1]) + got[2]))
            mo = {i: local_oproj(i) for i in FINAL_PRODUCTS}
            out_ref[0] = _join([_scomb(mo, k) + prev[k] for k in range(4)])

        def everything(_, carry):
            phase1()
            lax.fori_loop(1, 8, task, 0)
            final()
            return carry

        lax.fori_loop(0, jnp.minimum(me + 1, 1), everything, 0)

    return pl.pallas_call(
        body,
        out_shape=jax.ShapeDtypeStruct((1, SQ, D), f32),
        in_specs=[pl.BlockSpec(memory_space=pl.ANY)] * 5,
        out_specs=pl.BlockSpec(memory_space=pltpu.VMEM),
        scratch_shapes=[
            pltpu.VMEM((SQ, D), f32),
            pltpu.VMEM((2, D, G * DH), f32),
            pltpu.VMEM((H, SKV, DH), f32),
            pltpu.VMEM((H, SKV, DH), f32),
            pltpu.VMEM((2, G * DH, D), f32),
            pltpu.VMEM((4,) + UNIT, bf16),
            pltpu.VMEM((SQ, G * DH), f32),
            pltpu.VMEM((4, SQ, D), f32),
            pltpu.VMEM((4,) + UNIT, bf16),
            pltpu.VMEM((3,) + UNIT, bf16),
            pltpu.SemaphoreType.DMA((2,)),
            pltpu.SemaphoreType.DMA((G + 1,)),
            pltpu.SemaphoreType.DMA((G + 1,)),
            pltpu.SemaphoreType.DMA((G + 1,)),
            pltpu.SemaphoreType.DMA((4,)),
            pltpu.SemaphoreType.DMA,
            pltpu.SemaphoreType.DMA((3,)),
            pltpu.SemaphoreType.DMA,
            pltpu.SemaphoreType.DMA,
            pltpu.SemaphoreType.REGULAR,
        ],
        compiler_params=pltpu.CompilerParams(
            collective_id=0,
            disable_semaphore_checks=True,
            disable_bounds_checks=True,
            vmem_limit_bytes=100 * 1024 * 1024,
        ),
    )(x, Wq, K_ext, V_ext, Wo)
```

```python
import jax
import jax.numpy as jnp
from jax import lax
from jax.experimental import pallas as pl
from jax.experimental.pallas import tpu as pltpu

N_DEV = 4
SQ = 512
SKV = 2048
D = 1024
H = 8
G = 4
DH = 128
BQ = 256
PC = 64
UNIT = (2, 2, 2, PC, D)
QSCALE = 0.08838834764831843 * 1.4426950408889634

bf16 = jnp.bfloat16
f32 = jnp.float32

LOAD_ORDER = "x0 w0 k0 x1 w1 v0 k1 v1 w2 w3 k2 v2 k3 v3 u0 u1 u2"


def _scores(h):
    return f"s{h}a x{h}a s{h}b x{h}b12"


def _values(h):
    return f"o{h}a o{h}b12"


PHASE1 = (
    ("x0", "c0"), ("w0", "q0a g0"), ("k0", "s0a x0a"),
    ("x1", "c1 g1 q0b s0b x0b12"), ("w1", "q1"), ("v0", _values(0)),
    ("k1", _scores(1)), ("v1", _values(1)), ("w2 w3", "Q2"),
    ("k2", _scores(2)), ("v2", _values(2)), ("k3", _scores(3)),
    ("v3", _values(3)), ("u0 u1", "P2 P6 P5 P1"),
)
PHASE1_Q_ORDER = (2, 3, 6, 4, 5, 1, 7)
FINAL_PRODUCTS = (3, 7, 4)
TASK_PROG = ("Q5 Q7 Q3 Q4 Q1 Q2 A1b A3a Q6 A3b A1a A2b A0b A0a A2a "
             "O2 O3 O5 O4 O7 O6 O1")
TASK_SPLIT = (0, 8, 8, 12, 8, 12, 8, 0)
TASK_HINT = (0, 0, 1, 1, 1, 1, 2, 1)
TASK_NESTED = (2, 3, 6, 7)
LOCAL_NESTED = (1, 2, 5, 6)
INNER_ORDER = (1, 2, 4, 7, 5, 3, 6)


def _recip(l):
    r = pl.reciprocal(l, approx=True)
    return r * (2.0 - l * r)


def _mm(a, b):
    return jnp.dot(a.astype(bf16), b.astype(bf16), preferred_element_type=f32)


def _quarters(a):
    m, n = a.shape
    return (a[:m // 2, :n // 2], a[:m // 2, n // 2:],
            a[m // 2:, :n // 2], a[m // 2:, n // 2:])


def _join(c):
    return jnp.concatenate([jnp.concatenate(c[:2], axis=1),
                            jnp.concatenate(c[2:], axis=1)], axis=0)


_COMB = ({1: 1, 4: 1, 5: -1, 7: 1}, {3: 1, 5: 1}, {2: 1, 4: 1},
         {1: 1, 2: -1, 3: 1, 6: 1})
_B_USED = {1: (0, 3), 2: (0,), 3: (1, 3), 4: (0, 2), 5: (3,), 6: (0, 1),
           7: (2, 3)}


def _sprod(i, A, B, mm=_mm):
    b11, b12, b21, b22 = B

    def f(k):
        return A[k]().astype(f32)

    if i == 1:
        return mm(f(0) + f(3), b11 + b22)
    if i == 2:
        return mm(f(2) + f(3), b11)
    if i == 3:
        return mm(A[0](), b12 - b22)
    if i == 4:
        return mm(A[3](), b21 - b11)
    if i == 5:
        return mm(f(0) + f(1), b22)
    if i == 6:
        return mm(f(2) - f(0), b11 + b12)
    return mm(f(1) - f(3), b21 + b22)


def _scomb(M, k):
    terms = [(i, _COMB[k][i]) for i in M if i in _COMB[k]]
    if terms[0][1] < 0:
        terms[0], terms[1] = terms[1], terms[0]
    r = M[terms[0][0]]
    for i, sign in terms[1:]:
        r = r + M[i] if sign > 0 else r - M[i]
    return r


def _strassen(a, b, order):
    A = [lambda q=q: q for q in _quarters(a)]
    B = _quarters(b)
    M = {i: _sprod(i, A, B) for i in order}
    return [_scomb(M, k) for k in range(4)]


def _mm_nested(a, b):
    return _join(_strassen(a, b, INNER_ORDER))


def _tile_sum(p):
    r = p[:, 0:128]
    for c in range(1, p.shape[1] // 128):
        r = r + p[:, c * 128:(c + 1) * 128]
    return r


def _rowmax(s, sp):
    return jnp.max(s[:, :sp] if sp else s, axis=1, keepdims=True)


def pallas_dist_attn_cross_mha_kvrep_htp_ss_b1_sq512_skv2048_d1024_hq8_dh128_kernel(
    x: jax.Array,
    Wq: jax.Array,
    K_ext: jax.Array,
    V_ext: jax.Array,
    Wo: jax.Array,
):
    def body(x_hbm, wq_hbm, k_hbm, v_hbm, wo_hbm, out_ref,
             x_v, wq_v, k_v, v_v, wo_v, xg, o_loc, acc, ps, pr,
             x_sem, wq_sem, k_sem, v_sem, wo_sem,
             ag_send, ag_recv, rs_send, rs_recv, fence):
        me = lax.axis_index("i")
        right = lax.rem(me + 1, N_DEV)
        diag = lax.rem(me + 2, N_DEV)
        left = lax.rem(me + 3, N_DEV)
        h0 = me * H

        copy = pltpu.make_async_copy
        x_cp = [copy(x_hbm.at[0, pl.ds(j * BQ, BQ), :],
                     x_v.at[pl.ds(j * BQ, BQ), :], x_sem.at[j])
                for j in range(2)]
        wq_cp = [copy(wq_hbm.at[:, pl.ds(h * DH, DH)],
                      wq_v.at[0, :, pl.ds(h * DH, DH)], wq_sem.at[h])
                 for h in range(G)]
        wq_cp.append(copy(wq_hbm.at[:, pl.ds(G * DH, G * DH)], wq_v.at[1],
                          wq_sem.at[G]))
        k_cp = [copy(k_hbm.at[0, :, h0 + h, :], k_v.at[h], k_sem.at[min(h, G)])
                for h in range(H)]
        v_cp = [copy(v_hbm.at[0, :, h0 + h, :], v_v.at[h], v_sem.at[min(h, G)])
                for h in range(H)]
        wo_blocks = ((pl.ds(0, BQ), pl.ds(0, D)),
                     (pl.ds(BQ, BQ), pl.ds(D // 2, D // 2)),
                     (pl.ds(BQ, BQ), pl.ds(0, D // 2)))
        wo_cp = [copy(wo_hbm.at[r, c], wo_v.at[0, r, c], wo_sem.at[i])
                 for i, (r, c) in enumerate(wo_blocks)]
        wo_cp.append(copy(wo_hbm.at[pl.ds(G * DH, G * DH), :], wo_v.at[1],
                          wo_sem.at[3]))

        def start_in_order(copies):
            for c in copies:
                c.start()
                pl.semaphore_signal(fence, 1)
            pl.semaphore_wait(fence, len(copies))

        def wait_total(ref, sem):
            copy(ref, ref, sem).wait()

        def remote(src, dst, ssem, rsem, dev):
            return pltpu.make_async_remote_copy(
                src_ref=src, dst_ref=dst, send_sem=ssem, recv_sem=rsem,
                device_id=(dev,), device_id_type=pl.DeviceIdType.MESH)

        def ag_copies(u):
            return [remote(xg.at[0, c if u == 2 else u // 2], xg.at[u, :, :, c],
                           ag_send, ag_recv.at[u - 1],
                           diag if u == 2 else (right if c else left))
                    for c in range(2)]

        def rs_start(u):
            is_d = u == 2
            for c in range(2):
                slot = jnp.where(is_d, 2, c)
                half = jnp.where(is_d, c, lax.shift_right_logical(u, 1))
                dev = jnp.where(is_d, diag, left if c else right)
                remote(ps.at[u, :, :, c], pr.at[slot, half],
                       rs_send, rs_recv, dev).start()

        def rows_of(ref, *idx):
            v = ref[idx]
            return v.reshape(-1, D)

        def qk(qf, h):
            return lax.dot_general(qf.astype(bf16), k_v[h].astype(bf16),
                                   (((1,), (1,)), ((), ())),
                                   preferred_element_type=f32)

        def attend(s, h, sp, m1=None):
            vb = v_v[h].astype(bf16)
            if m1 is None:
                m1 = _rowmax(s, sp)
            if sp == 0:
                p = jnp.exp2(s - m1)
                lp = _tile_sum(p)
                o = jnp.dot(p.astype(bf16), vb, preferred_element_type=f32)
            else:
                p1 = jnp.exp2(s[:, :sp] - m1)
                o1 = jnp.dot(p1.astype(bf16), vb[:sp], preferred_element_type=f32)
                m = jnp.maximum(m1, jnp.max(s[:, sp:], axis=1, keepdims=True))
                p2 = jnp.exp2(s[:, sp:] - m)
                alpha = jnp.exp2(m1 - m)
                lp = _tile_sum(p1) * alpha + _tile_sum(p2)
                o = o1 * alpha + jnp.dot(p2.astype(bf16), vb[sp:],
                                         preferred_element_type=f32)
            return o * _recip(jnp.sum(lp, axis=1, keepdims=True)), lp

        def local_oproj(i):
            hd, hn = G * DH // 2, D // 2
            oa = [lambda j=j, c=c: o_loc[pl.ds(j * BQ, BQ), pl.ds(c * hd, hd)]
                  for j in range(2) for c in range(2)]
            wo4 = [wo_v[0, pl.ds(r * hd, hd), pl.ds(c * hn, hn)]
                   if 2 * r + c in _B_USED[i] else None
                   for r in range(2) for c in range(2)]
            return _sprod(i, oa, wo4, _mm_nested if i in LOCAL_NESTED else _mm)

        def phase1():
            cps = {"x": x_cp, "w": wq_cp, "k": k_cp, "v": v_cp, "u": wo_cp}
            order = [cps[w[0]][int(w[1])] for w in LOAD_ORDER.split()]
            order.append(wq_cp[G])
            for h in range(G, H):
                order += [k_cp[h], v_cp[h]]
            order.append(wo_cp[3])
            start_in_order(order)

            barrier = pltpu.get_barrier_semaphore()
            for peer in (right, diag, left):
                pl.semaphore_signal(barrier, inc=1, device_id=(peer,),
                                    device_id_type=pl.DeviceIdType.MESH)

            qs, ss, mx, mo = {}, {}, {}, {}
            for waits, ops in PHASE1:
                for w in waits.split():
                    cps[w[0]][int(w[1])].wait()
                for op in ops.split():
                    kind, h = op[0], int(op[1])
                    if kind == "c":
                        xg[0, h] = x_v[pl.ds(h * BQ, BQ), :].astype(
                            bf16).reshape(UNIT[1:])
                    elif kind == "g" and h == 0:
                        pl.semaphore_wait(barrier, 3)
                        start_in_order(ag_copies(1))
                    elif kind == "g":
                        start_in_order(ag_copies(2))
                    elif kind == "Q":
                        q4 = _strassen(rows_of(xg, 0), wq_v[0, :, h * DH:(h + 2) * DH],
                                       PHASE1_Q_ORDER)
                        for j in range(2):
                            for hh in range(2):
                                qs[h + hh, j] = q4[2 * j + hh] * QSCALE
                    elif kind == "q" and len(op) == 2:
                        q = _mm(rows_of(xg, 0), wq_v[0, :, h * DH:(h + 1) * DH]) * QSCALE
                        for j in range(2):
                            qs[h, j] = q[j * BQ:(j + 1) * BQ]
                    elif kind == "P":
                        mo[h] = local_oproj(h)
                    else:
                        j = "ab".index(op[2])
                        rows = pl.ds(j * BQ, BQ)
                        sp = int(op[3:] or 0) * 128
                        if kind == "q":
                            qs[h, j] = _mm(rows_of(xg, 0, j),
                                           wq_v[0, :, h * DH:(h + 1) * DH]) * QSCALE
                        elif kind == "s":
                            ss[h, j] = qk(qs[h, j], h)
                        elif kind == "x":
                            mx[h, j] = _rowmax(ss[h, j], sp)
                        else:
                            o_loc[rows, h * DH:(h + 1) * DH] = attend(
                                ss[h, j], h, sp, mx[h, j])[0]
            acc[0] = _join([_scomb(mo, k) for k in range(4)])
            wo_cp[2].wait()

        def task(t, carry):
            u = lax.shift_right_logical(t + 1, 1) & 3
            g = ((t + 1) & 1) | lax.shift_right_logical(t + 1, 3)

            @pl.when(g == 0)
            def _():
                wait_total(xg.at[u], ag_recv.at[u - 1])

            @pl.when(t == 2)
            def _():
                wq_cp[G].wait()
                wait_total(k_v.at[pl.ds(G, G)], k_sem.at[G])
                wait_total(v_v.at[pl.ds(G, G)], v_sem.at[G])
                wo_cp[3].wait()

            xq = _quarters(rows_of(xg, u))
            xa = [lambda k=k: xq[k] for k in range(4)]
            wq4 = _quarters(wq_v[g])
            wo4 = _quarters(wo_v[g])
            prev = _quarters(jnp.where(g == 1, acc[u], 0.0))
            mq, mo, q4, oo, lps = {}, {}, {}, {}, []
            oa = [lambda j=j, c=c: jnp.concatenate(
                      [oo[j, 2 * c], oo[j, 2 * c + 1]], axis=1)
                  for j in range(2) for c in range(2)]
            for op in TASK_PROG.split():
                i = int(op[1])
                if op[0] == "Q":
                    mq[i] = _sprod(i, xa, wq4)
                elif op[0] == "O":
                    mo[i] = _sprod(i, oa, wo4,
                                   _mm_nested if i in TASK_NESTED else _mm)
                else:
                    j = "ab".index(op[2])
                    k = 2 * j + i // 2
                    if k not in q4:
                        q4[k] = _scomb(mq, k)
                    qf = q4[k][:, (i % 2) * DH:(i % 2 + 1) * DH] * QSCALE
                    lag = TASK_HINT[len(lps)]
                    if lag:
                        qf = qf + 0.0 * lps[-lag]
                    oo[j, i], lp = attend(qk(qf, g * G + i), g * G + i,
                                          TASK_SPLIT[len(lps)] * 128)
                    lps.append(lp)
            res = _join([_scomb(mo, k) + prev[k] for k in range(4)])
            acc[u] = res
            ps[u] = res.astype(bf16).reshape(UNIT)

            @pl.when(jnp.logical_and(g == 1, u > 0))
            def _():
                rs_start(u)

            @pl.when(t == 1)
            def _():
                for c in ag_copies(3):
                    c.start()

            return carry

        def final():
            wait_total(pr, rs_recv)
            wait_total(xg.at[pl.ds(1, 3)], ag_send)
            wait_total(ps.at[pl.ds(1, 3)], rs_send)
            got = [rows_of(pr, i).astype(f32) for i in range(3)]
            prev = _quarters(acc[0] + ((got[0] + got[1]) + got[2]))
            mo = {i: local_oproj(i) for i in FINAL_PRODUCTS}
            out_ref[0] = _join([_scomb(mo, k) + prev[k] for k in range(4)])

        def everything(_, carry):
            phase1()
            lax.fori_loop(1, 8, task, 0)
            final()
            return carry

        lax.fori_loop(0, jnp.minimum(me + 1, 1), everything, 0)

    return pl.pallas_call(
        body,
        out_shape=jax.ShapeDtypeStruct((1, SQ, D), f32),
        in_specs=[pl.BlockSpec(memory_space=pl.ANY)] * 5,
        out_specs=pl.BlockSpec(memory_space=pltpu.VMEM),
        scratch_shapes=[
            pltpu.VMEM((SQ, D), f32),
            pltpu.VMEM((2, D, G * DH), f32),
            pltpu.VMEM((H, SKV, DH), f32),
            pltpu.VMEM((H, SKV, DH), f32),
            pltpu.VMEM((2, G * DH, D), f32),
            pltpu.VMEM((4,) + UNIT, bf16),
            pltpu.VMEM((SQ, G * DH), f32),
            pltpu.VMEM((4, SQ, D), f32),
            pltpu.VMEM((4,) + UNIT, bf16),
            pltpu.VMEM((3,) + UNIT, bf16),
            pltpu.SemaphoreType.DMA((2,)),
            pltpu.SemaphoreType.DMA((G + 1,)),
            pltpu.SemaphoreType.DMA((G + 1,)),
            pltpu.SemaphoreType.DMA((G + 1,)),
            pltpu.SemaphoreType.DMA((4,)),
            pltpu.SemaphoreType.DMA,
            pltpu.SemaphoreType.DMA((3,)),
            pltpu.SemaphoreType.DMA,
            pltpu.SemaphoreType.DMA,
            pltpu.SemaphoreType.REGULAR,
        ],
        compiler_params=pltpu.CompilerParams(
            collective_id=0,
            disable_semaphore_checks=True,
            disable_bounds_checks=True,
            vmem_limit_bytes=100 * 1024 * 1024,
        ),
    )(x, Wq, K_ext, V_ext, Wo)
```

```python
import jax
import jax.numpy as jnp
from jax import lax
from jax.experimental import pallas as pl
from jax.experimental.pallas import tpu as pltpu

N_DEV = 4
SQ = 512
SKV = 2048
D = 1024
H = 8
G = 4
DH = 128
BQ = 256
PC = 64
UNIT = (2, 2, 2, PC, D)
QSCALE = 0.08838834764831843 * 1.4426950408889634

bf16 = jnp.bfloat16
f32 = jnp.float32

LOAD_ORDER = "x0 w0 k0 x1 w1 v0 k1 v1 w2 w3 k2 v2 k3 v3 u0 u1 u2"


def _scores(h):
    return f"s{h}a x{h}a s{h}b x{h}b12"


def _values(h):
    return f"o{h}a o{h}b12"


PHASE1 = (
    ("x0", "c0"), ("w0", "q0a g0"), ("k0", "s0a x0a"),
    ("x1", "c1 g1 q0b s0b x0b12"), ("w1", "q1"), ("v0", _values(0)),
    ("k1", _scores(1)), ("v1", _values(1)), ("w2 w3", "Q2"),
    ("k2", _scores(2)), ("v2", _values(2)), ("k3", _scores(3)),
    ("v3", _values(3)), ("u0 u1", "P2 P6 P5 P1"),
)
PHASE1_Q_ORDER = (2, 3, 6, 4, 5, 1, 7)
FINAL_PRODUCTS = (3, 7, 4)
TASK_PROG = ("Q5 Q7 Q3 Q4 Q1 Q2 A1b A3a Q6 A3b A1a A2b A0b A0a A2a "
             "O2 O3 O5 O4 O7 O6 O1")
TASK_SPLIT = (0, 8, 8, 12, 8, 12, 8, 0)
TASK_HINT = (0, 0, 1, 1, 1, 1, 2, 1)
TASK_NESTED = (2, 3, 6, 7)
LOCAL_NESTED = (1, 2, 5, 6)
INNER_ORDER = (1, 2, 4, 7, 5, 3, 6)


def _recip(l):
    r = pl.reciprocal(l, approx=True)
    return r * (2.0 - l * r)


def _mm(a, b):
    return jnp.dot(a.astype(bf16), b.astype(bf16), preferred_element_type=f32)


def _quarters(a):
    m, n = a.shape
    return (a[:m // 2, :n // 2], a[:m // 2, n // 2:],
            a[m // 2:, :n // 2], a[m // 2:, n // 2:])


def _join(c):
    return jnp.concatenate([jnp.concatenate(c[:2], axis=1),
                            jnp.concatenate(c[2:], axis=1)], axis=0)


_COMB = ({1: 1, 4: 1, 5: -1, 7: 1}, {3: 1, 5: 1}, {2: 1, 4: 1},
         {1: 1, 2: -1, 3: 1, 6: 1})
_B_USED = {1: (0, 3), 2: (0,), 3: (1, 3), 4: (0, 2), 5: (3,), 6: (0, 1),
           7: (2, 3)}


def _sprod(i, A, B, mm=_mm):
    b11, b12, b21, b22 = B

    def f(k):
        return A[k]().astype(f32)

    if i == 1:
        return mm(f(0) + f(3), b11 + b22)
    if i == 2:
        return mm(f(2) + f(3), b11)
    if i == 3:
        return mm(A[0](), b12 - b22)
    if i == 4:
        return mm(A[3](), b21 - b11)
    if i == 5:
        return mm(f(0) + f(1), b22)
    if i == 6:
        return mm(f(2) - f(0), b11 + b12)
    return mm(f(1) - f(3), b21 + b22)


def _scomb(M, k):
    terms = [(i, _COMB[k][i]) for i in M if i in _COMB[k]]
    if terms[0][1] < 0:
        terms[0], terms[1] = terms[1], terms[0]
    r = M[terms[0][0]]
    for i, sign in terms[1:]:
        r = r + M[i] if sign > 0 else r - M[i]
    return r


def _strassen(a, b, order):
    A = [lambda q=q: q for q in _quarters(a)]
    B = _quarters(b)
    M = {i: _sprod(i, A, B) for i in order}
    return [_scomb(M, k) for k in range(4)]


def _mm_nested(a, b):
    return _join(_strassen(a, b, INNER_ORDER))


def _tile_sum(p):
    r = p[:, 0:128]
    for c in range(1, p.shape[1] // 128):
        r = r + p[:, c * 128:(c + 1) * 128]
    return r


def _rowmax(s, sp):
    return jnp.max(s[:, :sp] if sp else s, axis=1, keepdims=True)


def pallas_dist_attn_cross_mha_kvrep_htp_ss_b1_sq512_skv2048_d1024_hq8_dh128_kernel(
    x: jax.Array,
    Wq: jax.Array,
    K_ext: jax.Array,
    V_ext: jax.Array,
    Wo: jax.Array,
):
    def body(x_hbm, wq_hbm, k_hbm, v_hbm, wo_hbm, out_ref,
             x_v, wq_v, k_v, v_v, wo_v, xg, o_loc, acc, ps, pr,
             x_sem, wq_sem, k_sem, v_sem, wo_sem,
             ag_send, ag_recv, rs_send, rs_recv, fence):
        me = lax.axis_index("i")
        right = lax.rem(me + 1, N_DEV)
        diag = lax.rem(me + 2, N_DEV)
        left = lax.rem(me + 3, N_DEV)
        h0 = me * H

        copy = pltpu.make_async_copy
        x_cp = [copy(x_hbm.at[0, pl.ds(j * BQ, BQ), :],
                     x_v.at[pl.ds(j * BQ, BQ), :], x_sem.at[j])
                for j in range(2)]
        wq_cp = [copy(wq_hbm.at[:, pl.ds(h * DH, DH)],
                      wq_v.at[0, :, pl.ds(h * DH, DH)], wq_sem.at[h])
                 for h in range(G)]
        wq_cp.append(copy(wq_hbm.at[:, pl.ds(G * DH, G * DH)], wq_v.at[1],
                          wq_sem.at[G]))
        k_cp = [copy(k_hbm.at[0, :, h0 + h, :], k_v.at[h], k_sem.at[min(h, G)])
                for h in range(H)]
        v_cp = [copy(v_hbm.at[0, :, h0 + h, :], v_v.at[h], v_sem.at[min(h, G)])
                for h in range(H)]
        wo_blocks = ((pl.ds(0, BQ), pl.ds(0, D)),
                     (pl.ds(BQ, BQ), pl.ds(D // 2, D // 2)),
                     (pl.ds(BQ, BQ), pl.ds(0, D // 2)))
        wo_cp = [copy(wo_hbm.at[r, c], wo_v.at[0, r, c], wo_sem.at[i])
                 for i, (r, c) in enumerate(wo_blocks)]
        wo_cp.append(copy(wo_hbm.at[pl.ds(G * DH, G * DH), :], wo_v.at[1],
                          wo_sem.at[3]))

        def start_in_order(copies):
            for c in copies:
                c.start()
                pl.semaphore_signal(fence, 1)
            pl.semaphore_wait(fence, len(copies))

        def wait_total(ref, sem):
            copy(ref, ref, sem).wait()

        def remote(src, dst, ssem, rsem, dev):
            return pltpu.make_async_remote_copy(
                src_ref=src, dst_ref=dst, send_sem=ssem, recv_sem=rsem,
                device_id=(dev,), device_id_type=pl.DeviceIdType.MESH)

        def ag_copies(u):
            return [remote(xg.at[0, c if u == 2 else u // 2], xg.at[u, :, :, c],
                           ag_send.at[2 * (u - 1) + c], ag_recv.at[u - 1],
                           diag if u == 2 else (right if c else left))
                    for c in range(2)]

        def rs_copies(u):
            is_d = u == 2
            return [remote(ps.at[u, :, :, c],
                           pr.at[jnp.where(is_d, 2, c),
                                 jnp.where(is_d, c, jnp.where(u == 3, 1, 0))],
                           rs_send.at[2 * (u - 1) + c], rs_recv,
                           jnp.where(is_d, diag, left if c else right))
                    for c in range(2)]

        def rows_of(ref, *idx):
            v = ref[idx]
            return v.reshape(-1, D)

        def qk(qf, h):
            return lax.dot_general(qf.astype(bf16), k_v[h].astype(bf16),
                                   (((1,), (1,)), ((), ())),
                                   preferred_element_type=f32)

        def attend(s, h, sp, m1=None):
            vb = v_v[h].astype(bf16)
            if m1 is None:
                m1 = _rowmax(s, sp)
            if sp == 0:
                p = jnp.exp2(s - m1)
                lp = _tile_sum(p)
                o = jnp.dot(p.astype(bf16), vb, preferred_element_type=f32)
            else:
                p1 = jnp.exp2(s[:, :sp] - m1)
                o1 = jnp.dot(p1.astype(bf16), vb[:sp], preferred_element_type=f32)
                m = jnp.maximum(m1, jnp.max(s[:, sp:], axis=1, keepdims=True))
                p2 = jnp.exp2(s[:, sp:] - m)
                alpha = jnp.exp2(m1 - m)
                lp = _tile_sum(p1) * alpha + _tile_sum(p2)
                o = o1 * alpha + jnp.dot(p2.astype(bf16), vb[sp:],
                                         preferred_element_type=f32)
            return o * _recip(jnp.sum(lp, axis=1, keepdims=True)), lp

        def local_oproj(i):
            hd, hn = G * DH // 2, D // 2
            oa = [lambda j=j, c=c: o_loc[pl.ds(j * BQ, BQ), pl.ds(c * hd, hd)]
                  for j in range(2) for c in range(2)]
            wo4 = [wo_v[0, pl.ds(r * hd, hd), pl.ds(c * hn, hn)]
                   if 2 * r + c in _B_USED[i] else None
                   for r in range(2) for c in range(2)]
            return _sprod(i, oa, wo4, _mm_nested if i in LOCAL_NESTED else _mm)

        def phase1():
            cps = {"x": x_cp, "w": wq_cp, "k": k_cp, "v": v_cp, "u": wo_cp}
            order = [cps[w[0]][int(w[1])] for w in LOAD_ORDER.split()]
            order.append(wq_cp[G])
            for h in range(G, H):
                order += [k_cp[h], v_cp[h]]
            order.append(wo_cp[3])
            start_in_order(order)

            barrier = pltpu.get_barrier_semaphore()
            for peer in (right, diag, left):
                pl.semaphore_signal(barrier, inc=1, device_id=(peer,),
                                    device_id_type=pl.DeviceIdType.MESH)

            qs, ss, mx, mo = {}, {}, {}, {}
            for waits, ops in PHASE1:
                for w in waits.split():
                    cps[w[0]][int(w[1])].wait()
                for op in ops.split():
                    kind, h = op[0], int(op[1])
                    if kind == "c":
                        xg[0, h] = x_v[pl.ds(h * BQ, BQ), :].astype(
                            bf16).reshape(UNIT[1:])
                    elif kind == "g" and h == 0:
                        pl.semaphore_wait(barrier, 3)
                        start_in_order(ag_copies(1))
                    elif kind == "g":
                        start_in_order(ag_copies(2))
                    elif kind == "Q":
                        q4 = _strassen(rows_of(xg, 0), wq_v[0, :, h * DH:(h + 2) * DH],
                                       PHASE1_Q_ORDER)
                        for j in range(2):
                            for hh in range(2):
                                qs[h + hh, j] = q4[2 * j + hh] * QSCALE
                    elif kind == "q" and len(op) == 2:
                        q = _mm(rows_of(xg, 0), wq_v[0, :, h * DH:(h + 1) * DH]) * QSCALE
                        for j in range(2):
                            qs[h, j] = q[j * BQ:(j + 1) * BQ]
                    elif kind == "P":
                        mo[h] = local_oproj(h)
                    else:
                        j = "ab".index(op[2])
                        rows = pl.ds(j * BQ, BQ)
                        sp = int(op[3:] or 0) * 128
                        if kind == "q":
                            qs[h, j] = _mm(rows_of(xg, 0, j),
                                           wq_v[0, :, h * DH:(h + 1) * DH]) * QSCALE
                        elif kind == "s":
                            ss[h, j] = qk(qs[h, j], h)
                        elif kind == "x":
                            mx[h, j] = _rowmax(ss[h, j], sp)
                        else:
                            o_loc[rows, h * DH:(h + 1) * DH] = attend(
                                ss[h, j], h, sp, mx[h, j])[0]
            acc[0] = _join([_scomb(mo, k) for k in range(4)])
            wo_cp[2].wait()

        def task(t, carry):
            u = lax.shift_right_logical(t + 1, 1) & 3
            g = ((t + 1) & 1) | lax.shift_right_logical(t + 1, 3)

            @pl.when(g == 0)
            def _():
                wait_total(xg.at[u], ag_recv.at[u - 1])

            @pl.when(t == 2)
            def _():
                wq_cp[G].wait()
                wait_total(k_v.at[pl.ds(G, G)], k_sem.at[G])
                wait_total(v_v.at[pl.ds(G, G)], v_sem.at[G])
                wo_cp[3].wait()

            xq = _quarters(rows_of(xg, u))
            xa = [lambda k=k: xq[k] for k in range(4)]
            wq4 = _quarters(wq_v[g])
            wo4 = _quarters(wo_v[g])
            prev = _quarters(jnp.where(g == 1, acc[u], 0.0))
            mq, mo, q4, oo, lps = {}, {}, {}, {}, []
            oa = [lambda j=j, c=c: jnp.concatenate(
                      [oo[j, 2 * c], oo[j, 2 * c + 1]], axis=1)
                  for j in range(2) for c in range(2)]
            for op in TASK_PROG.split():
                i = int(op[1])
                if op[0] == "Q":
                    mq[i] = _sprod(i, xa, wq4)
                elif op[0] == "O":
                    mo[i] = _sprod(i, oa, wo4,
                                   _mm_nested if i in TASK_NESTED else _mm)
                else:
                    j = "ab".index(op[2])
                    k = 2 * j + i // 2
                    if k not in q4:
                        q4[k] = _scomb(mq, k)
                    qf = q4[k][:, (i % 2) * DH:(i % 2 + 1) * DH] * QSCALE
                    lag = TASK_HINT[len(lps)]
                    if lag:
                        qf = qf + 0.0 * lps[-lag]
                    oo[j, i], lp = attend(qk(qf, g * G + i), g * G + i,
                                          TASK_SPLIT[len(lps)] * 128)
                    lps.append(lp)
            res = _join([_scomb(mo, k) + prev[k] for k in range(4)])
            acc[u] = res
            ps[u] = res.astype(bf16).reshape(UNIT)

            @pl.when(jnp.logical_and(g == 1, u > 0))
            def _():
                for c in rs_copies(u):
                    c.start()

            @pl.when(t == 1)
            def _():
                for c in ag_copies(3):
                    c.start()

            return carry

        def final():
            wait_total(pr, rs_recv)
            for u in (1, 2, 3):
                for c in ag_copies(u) + rs_copies(u):
                    c.wait_send()
            got = [rows_of(pr, i).astype(f32) for i in range(3)]
            prev = _quarters(acc[0] + ((got[0] + got[1]) + got[2]))
            mo = {i: local_oproj(i) for i in FINAL_PRODUCTS}
            out_ref[0] = _join([_scomb(mo, k) + prev[k] for k in range(4)])

        def everything(i, carry):
            @pl.when(i == 0)
            def _():
                phase1()
                lax.fori_loop(1, 8, task, 0)
                final()

            return carry

        lax.fori_loop(0, 2, everything, 0)

    return pl.pallas_call(
        body,
        out_shape=jax.ShapeDtypeStruct((1, SQ, D), f32),
        in_specs=[pl.BlockSpec(memory_space=pl.ANY)] * 5,
        out_specs=pl.BlockSpec(memory_space=pltpu.VMEM),
        scratch_shapes=[
            pltpu.VMEM((SQ, D), f32),
            pltpu.VMEM((2, D, G * DH), f32),
            pltpu.VMEM((H, SKV, DH), f32),
            pltpu.VMEM((H, SKV, DH), f32),
            pltpu.VMEM((2, G * DH, D), f32),
            pltpu.VMEM((4,) + UNIT, bf16),
            pltpu.VMEM((SQ, G * DH), f32),
            pltpu.VMEM((4, SQ, D), f32),
            pltpu.VMEM((4,) + UNIT, bf16),
            pltpu.VMEM((3,) + UNIT, bf16),
            pltpu.SemaphoreType.DMA((2,)),
            pltpu.SemaphoreType.DMA((G + 1,)),
            pltpu.SemaphoreType.DMA((G + 1,)),
            pltpu.SemaphoreType.DMA((G + 1,)),
            pltpu.SemaphoreType.DMA((4,)),
            pltpu.SemaphoreType.DMA((6,)),
            pltpu.SemaphoreType.DMA((3,)),
            pltpu.SemaphoreType.DMA((6,)),
            pltpu.SemaphoreType.DMA,
            pltpu.SemaphoreType.REGULAR,
        ],
        compiler_params=pltpu.CompilerParams(
            collective_id=0,
            disable_semaphore_checks=True,
            disable_bounds_checks=True,
            vmem_limit_bytes=100 * 1024 * 1024,
        ),
    )(x, Wq, K_ext, V_ext, Wo)
```
